```python
import numpy as np

kernel_name = "dist_sort_i_m128_n64"

def setup_inputs():
    return {"x": np.random.randn(512, 64).astype(np.float32)}

def reference(x: np.ndarray) -> np.ndarray:
    return np.sort(x, axis=0)
```

```python
import jax
import jax.numpy as jnp
from jax import lax
from jax.experimental import pallas as pl
from jax.experimental.pallas import tpu as pltpu

N_DEV = 4
F32 = jnp.float32
BF16 = jnp.bfloat16
U32 = jnp.uint32
MESH = pl.DeviceIdType.MESH
SCOPES = False

_NET16 = (
    ((0, 13), (1, 12), (2, 15), (3, 14), (4, 8), (5, 6), (7, 11), (9, 10)),
    ((0, 5), (1, 7), (2, 9), (3, 4), (6, 13), (8, 14), (10, 15), (11, 12)),
    ((0, 1), (2, 3), (4, 5), (6, 8), (7, 9), (10, 11), (12, 13), (14, 15)),
    ((0, 2), (1, 3), (4, 10), (5, 11), (6, 7), (8, 9), (12, 14), (13, 15)),
    ((1, 2), (3, 12), (4, 6), (5, 7), (8, 10), (9, 11), (13, 14)),
    ((1, 4), (2, 6), (5, 8), (7, 10), (9, 13), (11, 14)),
    ((2, 4), (3, 6), (9, 12), (11, 13)),
    ((3, 5), (6, 8), (7, 9), (10, 12)),
    ((3, 4), (5, 6), (7, 8), (9, 10), (11, 12)),
    ((6, 7), (8, 9)),
)


def _scoped(name, fn):
    if SCOPES:
        with jax.named_scope(name):
            fn()
    else:
        fn()


def _roll(x, s):
    return pltpu.roll(x, s, axis=0)


def _vstage(y, bit, first, second):
    out = list(y)
    for v in range(len(y)):
        if not v & bit:
            out[v] = first(y[v], y[v | bit])
            out[v | bit] = second(y[v], y[v | bit])
    return out


def _sstage(x, d, low, first, second):
    if d == 4:
        r = _roll(x, 4)
        return jnp.where(low[4], first(x, r), second(x, r))
    return jnp.where(low[d], first(x, _roll(x, 8 - d)), second(x, _roll(x, d)))


def _transpose(w, lhs):
    out = []
    for k in range(4):
        p = lax.dot_general(lhs[k], w, (((1,), (1,)), ((), ())), preferred_element_type=F32)
        out += [p[8 * j:8 * j + 8, :] for j in range(4)]
    return out


def pallas_dist_sort_i_m128_n64_kernel(x: jax.Array):
    xt = x.T

    def body(x_hbm, o_ref, xv, sbuf, rbuf, own, tab, in_sem, ssem, rsem, go):
        me = lax.axis_index("i")
        cp_in = pltpu.make_async_copy(x_hbm, xv, in_sem)
        cp_in.start()
        bar = pltpu.get_barrier_semaphore()

        def signal(sem, dst):
            pl.semaphore_signal(sem, inc=1, device_id=(dst,), device_id_type=MESH)

        @pl.when(me == 0)
        def _():
            for dst in (2, 1, 3):
                signal(bar, dst)

        @pl.when((me & 1) == 1)
        def _():
            for dst in (2, 0):
                signal(bar, dst)

        @pl.when(me == 2)
        def _():
            pl.semaphore_wait(bar, 3)
            for dst in (0, 1, 3):
                signal(go, dst)

        mx, mn = jnp.maximum, jnp.minimum
        sub = lax.broadcasted_iota(jnp.int32, (8, 128), 0)
        lane = lax.broadcasted_iota(jnp.int32, (8, 128), 1)
        low = {d: (sub & d) == 0 for d in (1, 2, 4)}
        lane_lo = lane < 64
        lane_even = (lane & 1) == 0
        row = lax.broadcasted_iota(jnp.int32, (32, 128), 0)
        col = lax.broadcasted_iota(jnp.int32, (32, 128), 1)
        pm = jnp.where((row & 1) == 0, 1.0, -1.0)
        eye = [jnp.where(row + 32 * k == col, 1.0, 0.0).astype(BF16) for k in range(4)]
        eye_pm = [jnp.where(row + 32 * k == col, pm, 0.0).astype(BF16) for k in range(4)]
        neg_inf = jnp.full((64, 128), -jnp.inf, F32)
        pos_inf = jnp.full((64, 128), jnp.inf, F32)
        tab[0] = neg_inf
        tab[1] = neg_inf
        tab[4] = pos_inf
        tab[5] = pos_inf

        _scoped("w_in", cp_in.wait)
        xf = xv[...]
        y = _transpose(jnp.concatenate([xf, xf], axis=0).astype(BF16), eye_pm)
        for layer in _NET16:
            for a, b in layer:
                y[a], y[b] = mx(y[a], y[b]), mn(y[a], y[b])

        def clean16(y):
            for bit in (8, 4, 2, 1):
                y = _vstage(y, bit, mx, mn)
            return y

        for v in range(8):
            a, pb = y[v], _roll(y[15 - v], 4)
            hi, lo = mx(a, pb), mn(a, pb)
            y[v] = jnp.where(low[4], hi, lo)
            y[15 - v] = _roll(jnp.where(low[4], lo, hi), 4)
        y = clean16(y)
        y = [jnp.where(low[2], mx(y[v], _roll(y[15 - v], 2)), mn(y[v], _roll(y[15 - v], 6)))
             for v in range(16)]
        y = [_sstage(t, 4, low, mx, mn) for t in y]
        y = clean16(y)
        ua = [jnp.where(low[1], y[v], _roll(y[v + 8], 1)) for v in range(8)]
        ub = [-jnp.where(low[1], _roll(y[v], 7), y[v + 8]) for v in range(8)]

        def finish_half(h, half):
            for d in (2, 4, 1):
                h = [_sstage(t, d, low, mx, mn) for t in h]
            for bit in (4, 2, 1):
                h = _vstage(h, bit, mx, mn)
            dn = [jnp.where(lane_lo, h[2 * q], h[2 * q + 1]) for q in range(4)]
            for q in range(2):
                w = pltpu.bitcast(dn[2 * q + 1], U32) | (pltpu.bitcast(dn[2 * q], U32) >> 16)
                sbuf[half, pl.ds(q, 8, stride=2), :] = w
            return h

        def copy(k, slot, dst):
            return pltpu.make_async_remote_copy(
                src_ref=sbuf, dst_ref=rbuf.at[slot], send_sem=ssem.at[k],
                recv_sem=rsem.at[slot], device_id=(dst,), device_id_type=MESH)

        def copy_half(half, dst):
            return pltpu.make_async_remote_copy(
                src_ref=sbuf.at[half], dst_ref=rbuf.at[2, half], send_sem=ssem.at[2 + half],
                recv_sem=rsem.at[2 + half], device_id=(dst,), device_id_type=MESH)

        h_lo = finish_half([mn(a, b) for a, b in zip(ua, ub)], 1)

        @pl.when(me == 2)
        def _():
            copy_half(1, 0).start()

        h_hi = finish_half([mx(a, b) for a, b in zip(ua, ub)], 0)

        @pl.when(me == 2)
        def _():
            copy_half(0, 0).start()
            copy(0, 1, 3).start()
            copy(1, 1, 1).start()

        @pl.when((me & 1) == 1)
        def _():
            slot = me >> 1
            _scoped("w_bar", lambda: pl.semaphore_wait(bar, 1))
            copy(0, slot, 0).start()
            _scoped("w_go", lambda: pl.semaphore_wait(go, 1))
            copy_half(1, 4 - me).start()
            copy_half(0, 4 - me).start()
            copy(1, slot, 2).start()

        @pl.when(me == 0)
        def _():
            _scoped("w_bar", lambda: pl.semaphore_wait(bar, 2))
            copy(0, 0, 1).start()
            copy(1, 0, 3).start()
            _scoped("w_go", lambda: pl.semaphore_wait(go, 1))
            copy_half(1, 2).start()
            copy_half(0, 2).start()

        for half, h in ((0, h_hi), (1, h_lo)):
            for q in range(4):
                own[half, pl.ds(3 - q, 8, stride=4), :] = jnp.where(lane_lo, h[2 * q + 1], h[2 * q])
        ow = [None] * 8
        for half in range(2):
            for b4 in range(2):
                for b5 in range(2):
                    t = own[half, pl.ds(16 * b4 + 8 * b5, 8), :]
                    ow[7 - (4 * half + 2 * b5 + b4)] = _roll(t, 4)

        def load_half(slot, half):
            out = [None] * 4
            for b4 in range(2):
                t = pltpu.bitcast(rbuf[slot, half, pl.ds(8 * b4, 8), :], BF16).astype(F32)
                out[b4] = t[0:8]
                out[2 + b4] = t[8:16]
            return out

        def load_list(slot):
            return load_half(slot, 0) + load_half(slot, 1)

        def clean6(z):
            for bit in (4, 2, 1):
                z = _vstage(z, bit, mn, mx)
            for d in (4, 2, 1):
                z = [_sstage(t, d, low, mn, mx) for t in z]
            return z

        def clean7(z):
            z = clean6(z)
            r = [pltpu.roll(t, 64, axis=1) for t in z]
            return [jnp.where(lane_lo, mn(a, b), mx(a, b)) for a, b in zip(z, r)]

        def emit(z):
            z = clean6(z)
            ws = []
            for t in z:
                bits = pltpu.bitcast(t, U32)
                ws.append(pltpu.bitcast(bits | (bits >> 16), BF16))
            e = _transpose(jnp.concatenate(ws, axis=0), eye)
            for k in range(8):
                o_ref[pl.ds(8 * k, 8), :] = jnp.where(
                    lane_even, mn(e[k], e[k + 8]), mx(e[k], e[k + 8]))

        _scoped("w_n1", copy(0, 0, me).wait_recv)
        n1 = load_list(0)
        b0 = clean7([mn(a, b) for a, b in zip(ow, n1)])
        b1 = clean7([mx(a, b) for a, b in zip(ow, n1)])
        for k in range(8):
            tab[2, pl.ds(8 * k, 8), :] = b0[k]
            tab[3, pl.ds(8 * k, 8), :] = b1[k]
        _scoped("w_n2", copy(0, 1, me).wait_recv)
        n2 = load_list(1)
        ta = [tab[me, pl.ds(8 * k, 8), :] for k in range(8)]
        tb = [tab[me + 1, pl.ds(8 * k, 8), :] for k in range(8)]
        tc = [tab[me + 2, pl.ds(8 * k, 8), :] for k in range(8)]
        s_lo = clean7([mn(mx(u, a), b) for u, a, b in zip(n2, ta, tb)])
        s_hi = clean7([mn(mx(u, a), b) for u, a, b in zip(n2, tb, tc)])
        for k in range(2):
            copy(k, 0, me).wait_send()
            copy_half(k, me).wait_send()

        def full():
            u = load_list(2)
            emit([mn(mx(t, a), b) for t, a, b in zip(u, s_lo, s_hi)])

        _scoped("w_u", copy_half(1, me).wait_recv)

        @pl.when(me == 0)
        def _():
            ul = load_half(2, 1)
            bad = jnp.max(jnp.where(ul[0][0:1] < s_hi[4][0:1], 1.0, 0.0))
            emit(s_hi[:4] + [mn(t, b) for t, b in zip(ul, s_hi[4:])])
            _scoped("w_u2", copy_half(0, me).wait_recv)
            pl.when(bad > 0.0)(full)

        @pl.when(me != 0)
        def _():
            _scoped("w_u2", copy_half(0, me).wait_recv)
            full()

    out = pl.pallas_call(
        body,
        out_shape=jax.ShapeDtypeStruct((64, 128), F32),
        in_specs=[pl.BlockSpec(memory_space=pl.ANY)],
        out_specs=pl.BlockSpec(memory_space=pltpu.VMEM),
        scratch_shapes=[
            pltpu.VMEM((64, 128), F32),
            pltpu.VMEM((2, 16, 128), U32),
            pltpu.VMEM((3, 2, 16, 128), U32),
            pltpu.VMEM((2, 32, 128), F32),
            pltpu.VMEM((6, 64, 128), F32),
            pltpu.SemaphoreType.DMA,
            pltpu.SemaphoreType.DMA((4,)),
            pltpu.SemaphoreType.DMA((4,)),
            pltpu.SemaphoreType.REGULAR,
        ],
        compiler_params=pltpu.CompilerParams(collective_id=0, disable_semaphore_checks=True),
    )(xt)
    return out.T
```

```python
import jax
import jax.numpy as jnp
from jax import lax
from jax.experimental import pallas as pl
from jax.experimental.pallas import tpu as pltpu

F32 = jnp.float32
BF16 = jnp.bfloat16
U32 = jnp.uint32
MESH = pl.DeviceIdType.MESH

SKIP = 3
HEAD = 64 - 4 * SKIP

_NET16 = (
    ((0, 13), (1, 12), (2, 15), (3, 14), (4, 8), (5, 6), (7, 11), (9, 10)),
    ((0, 5), (1, 7), (2, 9), (3, 4), (6, 13), (8, 14), (10, 15), (11, 12)),
    ((0, 1), (2, 3), (4, 5), (6, 8), (7, 9), (10, 11), (12, 13), (14, 15)),
    ((0, 2), (1, 3), (4, 10), (5, 11), (6, 7), (8, 9), (12, 14), (13, 15)),
    ((1, 2), (3, 12), (4, 6), (5, 7), (8, 10), (9, 11), (13, 14)),
    ((1, 4), (2, 6), (5, 8), (7, 10), (9, 13), (11, 14)),
    ((2, 4), (3, 6), (9, 12), (11, 13)),
    ((3, 5), (6, 8), (7, 9), (10, 12)),
    ((3, 4), (5, 6), (7, 8), (9, 10), (11, 12)),
    ((6, 7), (8, 9)),
)
_ARRIVAL = (0, 4, 8, 12, 1, 5, 9, 13, 2, 6, 10, 14, 3, 7, 11, 15)
_WIRES = (0, 13, 5, 6, 1, 12, 7, 11, 2, 15, 9, 10, 3, 14, 4, 8)


def _roll(x, s):
    return pltpu.roll(x, s, axis=0)


def _vstage(y, bit, first, second):
    out = list(y)
    for v in range(len(y)):
        if not v & bit:
            out[v] = first(y[v], y[v | bit])
            out[v | bit] = second(y[v], y[v | bit])
    return out


def _sstage(x, d, low, first, second):
    if d == 4:
        r = _roll(x, 4)
        return jnp.where(low[4], first(x, r), second(x, r))
    return jnp.where(low[d], first(x, _roll(x, 8 - d)), second(x, _roll(x, d)))


def _split(a, b, d, low):
    if d == 4:
        return jnp.where(low[4], a, b), _roll(jnp.where(low[4], b, a), 4)
    return jnp.where(low[d], a, _roll(b, d)), jnp.where(low[d], _roll(a, 8 - d), b)


def _xstage(y, d, bit, low, first, second):
    out = list(y)
    for v in range(len(y)):
        if not v & bit:
            u, w = _split(y[v], y[v | bit], d, low)
            out[v] = first(u, w)
            out[v | bit] = second(u, w)
    return out


def _transpose(w, lhs):
    out = []
    for blk in lhs:
        p = lax.dot_general(blk, w, (((1,), (1,)), ((), ())), preferred_element_type=F32)
        out += [p[8 * j:8 * j + 8, :] for j in range(4)]
    return out


def _load_list(ref):
    out = []
    for m in range(ref.shape[0] // 8):
        t = pltpu.bitcast(ref[pl.ds(8 * m, 8), :], BF16).astype(F32)
        out += [t[0:8], t[8:16]]
    return out


def _body(x_hbm, o_ref, xv, sbuf, rbuf, fbuf, own, tab, in_sem, ssem, rsem, go):
    me = lax.axis_index("i")
    cp_in = pltpu.make_async_copy(x_hbm, xv, in_sem)
    cp_in.start()

    bar = pltpu.get_barrier_semaphore()

    def signal(sem, dst):
        pl.semaphore_signal(sem, inc=1, device_id=(dst,), device_id_type=MESH)

    @pl.when(me == 0)
    def _():
        for dst in (2, 1, 3):
            signal(bar, dst)

    @pl.when((me & 1) == 1)
    def _():
        for dst in (2, 0):
            signal(bar, dst)

    mx, mn = jnp.maximum, jnp.minimum
    sub = lax.broadcasted_iota(jnp.int32, (8, 128), 0)
    lane = lax.broadcasted_iota(jnp.int32, (8, 128), 1)
    low = {d: (sub & d) == 0 for d in (1, 2, 4)}
    lane_lo = lane < 64
    lane_even = (lane & 1) == 0
    row = lax.broadcasted_iota(jnp.int32, (32, 128), 0)
    col = lax.broadcasted_iota(jnp.int32, (32, 128), 1)
    pm = jnp.where((row & 1) == 0, 1.0, -1.0)
    eye = [jnp.where(row + 32 * k == col, 1.0, 0.0).astype(BF16) for k in (0, 2, 1, 3)]
    eye_pm = [jnp.where(row + 32 * k == col, pm, 0.0).astype(BF16) for k in range(4)]
    tab[0] = jnp.full((64, 128), -jnp.inf, F32)
    tab[1] = jnp.full((64, 128), -jnp.inf, F32)
    tab[4] = jnp.full((64, 128), jnp.inf, F32)
    tab[5] = jnp.full((64, 128), jnp.inf, F32)
    fbuf[pl.ds(0, SKIP), :] = jnp.full((SKIP, 128), 0x7F807F80, U32)

    @pl.when(me == 2)
    def _():
        pl.semaphore_wait(bar, 3)
        for dst in (0, 1, 3):
            signal(go, dst)

    cp_in.wait()
    xf = xv[...]
    t = _transpose(jnp.concatenate([xf, xf], axis=0).astype(BF16), eye_pm)
    y = [None] * 16
    for a, wire in zip(_ARRIVAL, _WIRES):
        y[wire] = t[a]
    for layer in _NET16:
        for a, b in layer:
            y[a], y[b] = mx(y[a], y[b]), mn(y[a], y[b])
    for v in range(8):
        a, pb = y[v], _roll(y[15 - v], 4)
        hi, lo = mx(a, pb), mn(a, pb)
        y[v] = jnp.where(low[4], hi, lo)
        y[15 - v] = _roll(jnp.where(low[4], lo, hi), 4)
    for bit in (8, 4, 2, 1):
        y = _vstage(y, bit, mx, mn)
    t = list(y)
    for v in range(0, 16, 2):
        u = jnp.where(low[2], t[v], _roll(t[v + 1], 2))
        w = jnp.where(low[2], _roll(t[15 - v], 2), _roll(t[14 - v], 4))
        y[v], y[v + 1] = mx(u, w), mn(u, w)
    y = _xstage(y, 4, 1, low, mx, mn)
    for bit in (8, 4, 2):
        y = _vstage(y, bit, mx, mn)
    y = _xstage(y, 2, 2, low, mx, mn)
    ua, ub = [], []
    for v in (0, 1, 4, 5, 8, 9, 12, 13):
        u, w = _split(y[v], y[v + 2], 1, low)
        ua.append(u)
        ub.append(-w)

    def finish_half(h, half):
        h = [_sstage(r, 4, low, mx, mn) for r in h]
        for bit in (1, 4, 2):
            h = _vstage(h, bit, mx, mn)
        h = _xstage(h, 2, 1, low, mx, mn)
        h = _xstage(h, 1, 4, low, mx, mn)
        dn = [jnp.where(lane_lo, h[q], h[q + 4]) for q in range(4)]
        for q in range(2):
            w = pltpu.bitcast(dn[2 * q + 1], U32) | (pltpu.bitcast(dn[2 * q], U32) >> 16)
            sbuf[pl.ds(16 * half + q, 8, stride=2), :] = w
        return h

    def copy(k, slot, dst, src=sbuf):
        return pltpu.make_async_remote_copy(
            src_ref=src, dst_ref=rbuf.at[slot], send_sem=ssem.at[k],
            recv_sem=rsem.at[slot], device_id=(dst,), device_id_type=MESH)

    head = pltpu.make_async_remote_copy(
        src_ref=sbuf.at[pl.ds(16 + SKIP, 16 - SKIP)],
        dst_ref=fbuf.at[pl.ds(SKIP, 16 - SKIP)], send_sem=ssem.at[2],
        recv_sem=rsem.at[3], device_id=(0,), device_id_type=MESH)

    h_lo = finish_half([mn(a, b) for a, b in zip(ua, ub)], 1)

    @pl.when(me == 2)
    def _():
        head.start()

    h_hi = finish_half([mx(a, b) for a, b in zip(ua, ub)], 0)

    @pl.when(me == 2)
    def _():
        copy(0, 1, 3).start()
        copy(1, 1, 1).start()

    @pl.when((me & 1) == 1)
    def _():
        pl.semaphore_wait(bar, 1)
        copy(0, me >> 1, 0).start()
        pl.semaphore_wait(go, 1)
        copy(2, 2, 4 - me).start()
        copy(1, me >> 1, 2).start()

    @pl.when(me == 0)
    def _():
        pl.semaphore_wait(bar, 2)
        copy(0, 0, 1).start()
        copy(1, 0, 3).start()
        pl.semaphore_wait(go, 1)
        copy(2, 2, 2).start()

    for half, h in ((0, h_hi), (1, h_lo)):
        for q in range(4):
            own[half, pl.ds(3 - q, 8, stride=4), :] = jnp.where(lane_lo, h[q + 4], h[q])
    ow = [_roll(own[(7 - k) // 4, pl.ds(8 * ((7 - k) % 4), 8), :], 4) for k in range(8)]

    def clean6(z, bits=(4, 2, 1)):
        for bit in bits:
            z = _vstage(z, bit, mn, mx)
        for d in (4, 2, 1):
            z = [_sstage(r, d, low, mn, mx) for r in z]
        return z

    def clean7(z):
        z = clean6(z)
        r = [pltpu.roll(a, 64, axis=1) for a in z]
        return [jnp.where(lane_lo, mn(a, b), mx(a, b)) for a, b in zip(z, r)]

    def emit(z, bits=(4, 2, 1)):
        ws = []
        for r in clean6(z, bits):
            w = pltpu.bitcast(r, U32)
            ws.append(pltpu.bitcast(w | (w >> 16), BF16))
        e = _transpose(jnp.concatenate(ws, axis=0), eye)
        for k in range(8):
            e0, e1 = e[k + (k & 4)], e[k + (k & 4) + 4]
            o_ref[pl.ds(8 * k, 8), :] = jnp.where(lane_even, mn(e0, e1), mx(e0, e1))

    def block(ref):
        return [ref[pl.ds(8 * k, 8), :] for k in range(8)]

    copy(0, 0, me).wait_recv()
    n1 = _load_list(rbuf.at[0])
    b0 = clean7([mn(a, b) for a, b in zip(ow, n1)])
    b1 = clean7([mx(a, b) for a, b in zip(ow, n1)])
    for k in range(8):
        tab[2, pl.ds(8 * k, 8), :] = b0[k]
        tab[3, pl.ds(8 * k, 8), :] = b1[k]
    copy(0, 1, me).wait_recv()
    n2 = _load_list(rbuf.at[1])
    ta, tb, tc = block(tab.at[me]), block(tab.at[me + 1]), block(tab.at[me + 2])
    s_lo = clean7([mn(mx(u, a), b) for u, a, b in zip(n2, ta, tb)])
    s_hi = clean7([mn(mx(u, a), b) for u, a, b in zip(n2, tb, tc)])

    for k in range(2):
        copy(k, 0, me).wait_send()

    @pl.when(me == 2)
    def _():
        head.wait_send()

    @pl.when(me != 2)
    def _():
        copy(2, 0, me).wait_send()

    def head_too_short(u4, s4):
        hit = jnp.logical_and(u4 < s4, sub == 2 * SKIP)
        return jnp.max(jnp.where(hit, 1.0, 0.0)) > 0.0

    def full():
        copy(0, 2, me).wait_recv()
        u = _load_list(rbuf.at[2])
        emit([mn(mx(r, a), b) for r, a, b in zip(u, s_lo, s_hi)])
        return u

    @pl.when(me != 0)
    def _():
        u = full()

        @pl.when(me == 1)
        def _():
            s0 = clean7([mn(r, b) for r, b in zip(u, block(tab.at[2]))])

            @pl.when(head_too_short(_load_list(rbuf.at[1, pl.ds(16, 8)])[0], s0[4]))
            def _():
                fwd = copy(2, 2, 0, rbuf.at[1])
                fwd.start()
                fwd.wait_send()

    @pl.when(me == 0)
    def _():
        head.wait_recv()
        ul = _load_list(fbuf)
        redo = head_too_short(ul[0], s_hi[4])
        z = [mn(r, a) for r, a in zip(ul, s_hi[:4])]
        z += [mx(a, mn(r, b)) for r, a, b in zip(ul, s_hi[:4], s_hi[4:])]
        emit(z, (2, 1))

        @pl.when(redo)
        def _():
            full()


def pallas_dist_sort_i_m128_n64_kernel(x: jax.Array):
    out = pl.pallas_call(
        _body,
        out_shape=jax.ShapeDtypeStruct((64, 128), F32),
        in_specs=[pl.BlockSpec(memory_space=pl.ANY)],
        out_specs=pl.BlockSpec(memory_space=pltpu.VMEM),
        scratch_shapes=[
            pltpu.VMEM((64, 128), F32),
            pltpu.VMEM((32, 128), U32),
            pltpu.VMEM((3, 32, 128), U32),
            pltpu.VMEM((16, 128), U32),
            pltpu.VMEM((2, 32, 128), F32),
            pltpu.VMEM((6, 64, 128), F32),
            pltpu.SemaphoreType.DMA,
            pltpu.SemaphoreType.DMA((3,)),
            pltpu.SemaphoreType.DMA((4,)),
            pltpu.SemaphoreType.REGULAR,
        ],
        compiler_params=pltpu.CompilerParams(
            collective_id=0, disable_semaphore_checks=True),
    )(x.T)
    return out.T
```

```python
import jax
import jax.numpy as jnp
from jax import lax
from jax.experimental import pallas as pl
from jax.experimental.pallas import tpu as pltpu

F32 = jnp.float32
BF16 = jnp.bfloat16
U32 = jnp.uint32
MESH = pl.DeviceIdType.MESH

SKIP = 3
HEAD = 64 - 4 * SKIP

_NET16 = (
    ((0, 13), (1, 12), (2, 15), (3, 14), (4, 8), (5, 6), (7, 11), (9, 10)),
    ((0, 5), (1, 7), (2, 9), (3, 4), (6, 13), (8, 14), (10, 15), (11, 12)),
    ((0, 1), (2, 3), (4, 5), (6, 8), (7, 9), (10, 11), (12, 13), (14, 15)),
    ((0, 2), (1, 3), (4, 10), (5, 11), (6, 7), (8, 9), (12, 14), (13, 15)),
    ((1, 2), (3, 12), (4, 6), (5, 7), (8, 10), (9, 11), (13, 14)),
    ((1, 4), (2, 6), (5, 8), (7, 10), (9, 13), (11, 14)),
    ((2, 4), (3, 6), (9, 12), (11, 13)),
    ((3, 5), (6, 8), (7, 9), (10, 12)),
    ((3, 4), (5, 6), (7, 8), (9, 10), (11, 12)),
    ((6, 7), (8, 9)),
)
_ARRIVAL = (0, 4, 8, 12, 1, 5, 9, 13, 2, 6, 10, 14, 3, 7, 11, 15)
_WIRES = (0, 13, 5, 6, 1, 12, 7, 11, 2, 15, 9, 10, 3, 14, 4, 8)


def _roll(x, s):
    return pltpu.roll(x, s, axis=0)


def _vstage(y, bit, first, second):
    out = list(y)
    for v in range(len(y)):
        if not v & bit:
            out[v] = first(y[v], y[v | bit])
            out[v | bit] = second(y[v], y[v | bit])
    return out


def _sstage(x, d, low, first, second):
    if d == 4:
        r = _roll(x, 4)
        return jnp.where(low[4], first(x, r), second(x, r))
    return jnp.where(low[d], first(x, _roll(x, 8 - d)), second(x, _roll(x, d)))


def _split(a, b, d, low):
    if d == 4:
        return jnp.where(low[4], a, b), _roll(jnp.where(low[4], b, a), 4)
    return jnp.where(low[d], a, _roll(b, d)), jnp.where(low[d], _roll(a, 8 - d), b)


def _xstage(y, d, bit, low, first, second):
    out = list(y)
    for v in range(len(y)):
        if not v & bit:
            u, w = _split(y[v], y[v | bit], d, low)
            out[v] = first(u, w)
            out[v | bit] = second(u, w)
    return out


def _transpose(w, lhs):
    out = []
    for blk in lhs:
        p = lax.dot_general(blk, w, (((1,), (1,)), ((), ())), preferred_element_type=F32)
        out += [p[8 * j:8 * j + 8, :] for j in range(4)]
    return out


def _load_half(ref):
    out = []
    for m in range(2):
        t = pltpu.bitcast(ref[pl.ds(8 * m, 8), :], BF16).astype(F32)
        out += [t[0:8], t[8:16]]
    return out


def _load_list(ref):
    return _load_half(ref.at[0]) + _load_half(ref.at[1])


def _body(x_hbm, o_ref, xv, sbuf, rbuf, fbuf, own, tab, in_sem, ssem, rsem, go):
    me = lax.axis_index("i")
    cp_in = pltpu.make_async_copy(x_hbm, xv, in_sem)
    cp_in.start()

    bar = pltpu.get_barrier_semaphore()

    def signal(sem, dst):
        pl.semaphore_signal(sem, inc=1, device_id=(dst,), device_id_type=MESH)

    @pl.when(me == 0)
    def _():
        for dst in (2, 1, 3):
            signal(bar, dst)

    @pl.when((me & 1) == 1)
    def _():
        for dst in (2, 0):
            signal(bar, dst)

    mx, mn = jnp.maximum, jnp.minimum
    sub = lax.broadcasted_iota(jnp.int32, (8, 128), 0)
    lane = lax.broadcasted_iota(jnp.int32, (8, 128), 1)
    low = {d: (sub & d) == 0 for d in (1, 2, 4)}
    lane_lo = lane < 64
    lane_even = (lane & 1) == 0
    row = lax.broadcasted_iota(jnp.int32, (32, 128), 0)
    col = lax.broadcasted_iota(jnp.int32, (32, 128), 1)
    pm = jnp.where((row & 1) == 0, 1.0, -1.0)
    eye = [jnp.where(row + 32 * k == col, 1.0, 0.0).astype(BF16) for k in (0, 2, 1, 3)]
    eye_pm = [jnp.where(row + 32 * k == col, pm, 0.0).astype(BF16) for k in range(4)]
    tab[0] = jnp.full((64, 128), -jnp.inf, F32)
    tab[1] = jnp.full((64, 128), -jnp.inf, F32)
    tab[4] = jnp.full((64, 128), jnp.inf, F32)
    tab[5] = jnp.full((64, 128), jnp.inf, F32)
    fbuf[pl.ds(0, SKIP), :] = jnp.full((SKIP, 128), 0x7F807F80, U32)

    @pl.when(me == 2)
    def _():
        pl.semaphore_wait(bar, 3)
        for dst in (0, 1, 3):
            signal(go, dst)

    cp_in.wait()
    xf = xv[...]
    t = _transpose(jnp.concatenate([xf, xf], axis=0).astype(BF16), eye_pm)
    y = [None] * 16
    for a, wire in zip(_ARRIVAL, _WIRES):
        y[wire] = t[a]
    for layer in _NET16:
        for a, b in layer:
            y[a], y[b] = mx(y[a], y[b]), mn(y[a], y[b])
    for v in range(8):
        a, pb = y[v], _roll(y[15 - v], 4)
        hi, lo = mx(a, pb), mn(a, pb)
        y[v] = jnp.where(low[4], hi, lo)
        y[15 - v] = _roll(jnp.where(low[4], lo, hi), 4)
    for bit in (8, 4, 2, 1):
        y = _vstage(y, bit, mx, mn)
    t = list(y)
    for v in range(0, 16, 2):
        u = jnp.where(low[2], t[v], _roll(t[v + 1], 2))
        w = jnp.where(low[2], _roll(t[15 - v], 2), _roll(t[14 - v], 4))
        y[v], y[v + 1] = mx(u, w), mn(u, w)
    y = _xstage(y, 4, 1, low, mx, mn)
    for bit in (8, 4, 2):
        y = _vstage(y, bit, mx, mn)
    y = _xstage(y, 2, 2, low, mx, mn)
    ua, ub = [], []
    for v in (0, 1, 4, 5, 8, 9, 12, 13):
        u, w = _split(y[v], y[v + 2], 1, low)
        ua.append(u)
        ub.append(-w)

    def finish_half(h, half):
        h = [_sstage(r, 4, low, mx, mn) for r in h]
        for bit in (1, 4, 2):
            h = _vstage(h, bit, mx, mn)
        h = _xstage(h, 2, 1, low, mx, mn)
        h = _xstage(h, 1, 4, low, mx, mn)
        dn = [jnp.where(lane_lo, h[q], h[q + 4]) for q in range(4)]
        for q in range(2):
            w = pltpu.bitcast(dn[2 * q + 1], U32) | (pltpu.bitcast(dn[2 * q], U32) >> 16)
            sbuf[half, pl.ds(q, 8, stride=2), :] = w
        return h

    def copy(k, slot, dst, src=sbuf):
        return pltpu.make_async_remote_copy(
            src_ref=src, dst_ref=rbuf.at[slot], send_sem=ssem.at[k],
            recv_sem=rsem.at[slot], device_id=(dst,), device_id_type=MESH)

    head = pltpu.make_async_remote_copy(
        src_ref=sbuf.at[1, pl.ds(SKIP, 16 - SKIP)],
        dst_ref=fbuf.at[pl.ds(SKIP, 16 - SKIP)], send_sem=ssem.at[2],
        recv_sem=rsem.at[3], device_id=(0,), device_id_type=MESH)

    h_lo = finish_half([mn(a, b) for a, b in zip(ua, ub)], 1)

    @pl.when(me == 2)
    def _():
        head.start()

    h_hi = finish_half([mx(a, b) for a, b in zip(ua, ub)], 0)

    @pl.when(me == 2)
    def _():
        copy(0, 1, 3).start()
        copy(1, 1, 1).start()

    @pl.when((me & 1) == 1)
    def _():
        pl.semaphore_wait(bar, 1)
        copy(0, me >> 1, 0).start()
        pl.semaphore_wait(go, 1)
        copy(2, 2, 4 - me).start()
        copy(1, me >> 1, 2).start()

    @pl.when(me == 0)
    def _():
        pl.semaphore_wait(bar, 2)
        copy(0, 0, 1).start()
        copy(1, 0, 3).start()
        pl.semaphore_wait(go, 1)
        copy(2, 2, 2).start()

    for half, h in ((0, h_hi), (1, h_lo)):
        for q in range(4):
            own[half, pl.ds(3 - q, 8, stride=4), :] = jnp.where(lane_lo, h[q + 4], h[q])
    ow = [_roll(own[(7 - k) // 4, pl.ds(8 * ((7 - k) % 4), 8), :], 4) for k in range(8)]

    def clean6(z, bits=(4, 2, 1)):
        for bit in bits:
            z = _vstage(z, bit, mn, mx)
        for d in (4, 2, 1):
            z = [_sstage(r, d, low, mn, mx) for r in z]
        return z

    def clean7(z):
        z = clean6(z)
        r = [pltpu.roll(a, 64, axis=1) for a in z]
        return [jnp.where(lane_lo, mn(a, b), mx(a, b)) for a, b in zip(z, r)]

    def emit(z, bits=(4, 2, 1)):
        ws = []
        for r in clean6(z, bits):
            w = pltpu.bitcast(r, U32)
            ws.append(pltpu.bitcast(w | (w >> 16), BF16))
        e = _transpose(jnp.concatenate(ws, axis=0), eye)
        for k in range(8):
            e0, e1 = e[k + (k & 4)], e[k + (k & 4) + 4]
            o_ref[pl.ds(8 * k, 8), :] = jnp.where(lane_even, mn(e0, e1), mx(e0, e1))

    def block(ref):
        return [ref[pl.ds(8 * k, 8), :] for k in range(8)]

    copy(0, 0, me).wait_recv()
    n1 = _load_list(rbuf.at[0])
    b0 = clean7([mn(a, b) for a, b in zip(ow, n1)])
    b1 = clean7([mx(a, b) for a, b in zip(ow, n1)])
    for k in range(8):
        tab[2, pl.ds(8 * k, 8), :] = b0[k]
        tab[3, pl.ds(8 * k, 8), :] = b1[k]
    copy(0, 1, me).wait_recv()
    n2 = _load_list(rbuf.at[1])
    ta, tb, tc = block(tab.at[me]), block(tab.at[me + 1]), block(tab.at[me + 2])
    s_lo = clean7([mn(mx(u, a), b) for u, a, b in zip(n2, ta, tb)])
    s_hi = clean7([mn(mx(u, a), b) for u, a, b in zip(n2, tb, tc)])

    for k in range(2):
        copy(k, 0, me).wait_send()

    @pl.when(me == 2)
    def _():
        head.wait_send()

    @pl.when(me != 2)
    def _():
        copy(2, 0, me).wait_send()

    def head_too_short(u4, s4):
        hit = jnp.logical_and(u4 < s4, sub == 2 * SKIP)
        return jnp.max(jnp.where(hit, 1.0, 0.0)) > 0.0

    def full():
        copy(0, 2, me).wait_recv()
        u = _load_list(rbuf.at[2])
        emit([mn(mx(r, a), b) for r, a, b in zip(u, s_lo, s_hi)])
        return u

    @pl.when(me != 0)
    def _():
        u = full()

        @pl.when(me == 1)
        def _():
            s0 = clean7([mn(r, b) for r, b in zip(u, block(tab.at[2]))])

            @pl.when(head_too_short(_load_half(rbuf.at[1, 1])[0], s0[4]))
            def _():
                fwd = copy(2, 2, 0, rbuf.at[1])
                fwd.start()
                fwd.wait_send()

    @pl.when(me == 0)
    def _():
        head.wait_recv()
        ul = _load_half(fbuf)
        redo = head_too_short(ul[0], s_hi[4])
        z = [mn(r, a) for r, a in zip(ul, s_hi[:4])]
        z += [mx(a, mn(r, b)) for r, a, b in zip(ul, s_hi[:4], s_hi[4:])]
        emit(z, (2, 1))

        @pl.when(redo)
        def _():
            full()


def pallas_dist_sort_i_m128_n64_kernel(x: jax.Array):
    out = pl.pallas_call(
        _body,
        out_shape=jax.ShapeDtypeStruct((64, 128), F32),
        in_specs=[pl.BlockSpec(memory_space=pl.ANY)],
        out_specs=pl.BlockSpec(memory_space=pltpu.VMEM),
        scratch_shapes=[
            pltpu.VMEM((64, 128), F32),
            pltpu.VMEM((2, 16, 128), U32),
            pltpu.VMEM((3, 2, 16, 128), U32),
            pltpu.VMEM((16, 128), U32),
            pltpu.VMEM((2, 32, 128), F32),
            pltpu.VMEM((6, 64, 128), F32),
            pltpu.SemaphoreType.DMA,
            pltpu.SemaphoreType.DMA((3,)),
            pltpu.SemaphoreType.DMA((4,)),
            pltpu.SemaphoreType.REGULAR,
        ],
        compiler_params=pltpu.CompilerParams(
            collective_id=0, disable_semaphore_checks=True),
    )(x.T)
    return out.T
```

```python
import jax
import jax.numpy as jnp
from jax import lax
from jax.experimental import pallas as pl
from jax.experimental.pallas import tpu as pltpu

F32 = jnp.float32
BF16 = jnp.bfloat16
U32 = jnp.uint32
MESH = pl.DeviceIdType.MESH

SKIP = 3
HEAD = 64 - 4 * SKIP

BF16_MAX = 3.3895313892515355e38
BOOST = 1.0078125

_NET16 = (
    ((0, 13), (1, 12), (2, 15), (3, 14), (4, 8), (5, 6), (7, 11), (9, 10)),
    ((0, 5), (1, 7), (2, 9), (3, 4), (6, 13), (8, 14), (10, 15), (11, 12)),
    ((0, 1), (2, 3), (4, 5), (6, 8), (7, 9), (10, 11), (12, 13), (14, 15)),
    ((0, 2), (1, 3), (4, 10), (5, 11), (6, 7), (8, 9), (12, 14), (13, 15)),
    ((1, 2), (3, 12), (4, 6), (5, 7), (8, 10), (9, 11), (13, 14)),
    ((1, 4), (2, 6), (5, 8), (7, 10), (9, 13), (11, 14)),
    ((2, 4), (3, 6), (9, 12), (11, 13)),
    ((3, 5), (6, 8), (7, 9), (10, 12)),
    ((3, 4), (5, 6), (7, 8), (9, 10), (11, 12)),
    ((6, 7), (8, 9)),
)
_ARRIVAL = (0, 4, 8, 12, 1, 5, 9, 13, 2, 6, 10, 14, 3, 7, 11, 15)
_WIRES = (0, 13, 5, 6, 1, 12, 7, 11, 2, 15, 9, 10, 3, 14, 4, 8)


def _roll(x, s):
    return pltpu.roll(x, s, axis=0)


def _vstage(y, bit, first, second):
    out = list(y)
    for v in range(len(y)):
        if not v & bit:
            out[v] = first(y[v], y[v | bit])
            out[v | bit] = second(y[v], y[v | bit])
    return out


def _sstage(x, d, low, first, second):
    if d == 4:
        r = _roll(x, 4)
        return jnp.where(low[4], first(x, r), second(x, r))
    return jnp.where(low[d], first(x, _roll(x, 8 - d)), second(x, _roll(x, d)))


def _split(a, b, d, low):
    if d == 4:
        return jnp.where(low[4], a, b), _roll(jnp.where(low[4], b, a), 4)
    return jnp.where(low[d], a, _roll(b, d)), jnp.where(low[d], _roll(a, 8 - d), b)


def _xstage(y, d, bit, low, first, second):
    out = list(y)
    for v in range(len(y)):
        if not v & bit:
            u, w = _split(y[v], y[v | bit], d, low)
            out[v] = first(u, w)
            out[v | bit] = second(u, w)
    return out


def _transpose(w, lhs):
    out = []
    for blk in lhs:
        p = lax.dot_general(blk, w, (((1,), (1,)), ((), ())), preferred_element_type=F32)
        out += [p[8 * j:8 * j + 8, :] for j in range(4)]
    return out


def _load_half(ref):
    out = []
    for m in range(2):
        t = pltpu.bitcast(ref[pl.ds(8 * m, 8), :], BF16).astype(F32)
        out += [t[0:8], t[8:16]]
    return out


def _load_list(ref):
    return _load_half(ref.at[0]) + _load_half(ref.at[1])


def _body(x_hbm, o_ref, xv, sbuf, rbuf, fbuf, own, tab, in_sem, ssem, rsem, go):
    me = lax.axis_index("i")
    cp_in = pltpu.make_async_copy(x_hbm, xv, in_sem)
    cp_in.start()
    fbuf[pl.ds(0, SKIP), :] = jnp.full((SKIP, 128), 0x7F807F80, U32)

    bar = pltpu.get_barrier_semaphore()

    def signal(sem, dst):
        pl.semaphore_signal(sem, inc=1, device_id=(dst,), device_id_type=MESH)

    @pl.when(me == 0)
    def _():
        for dst in (2, 1, 3):
            signal(bar, dst)

    @pl.when((me & 1) == 1)
    def _():
        for dst in (2, 0):
            signal(bar, dst)

    mx, mn = jnp.maximum, jnp.minimum
    sub = lax.broadcasted_iota(jnp.int32, (8, 128), 0)
    lane = lax.broadcasted_iota(jnp.int32, (8, 128), 1)
    low = {d: (sub & d) == 0 for d in (1, 2, 4)}
    lane_lo = lane < 64
    lane_even = (lane & 1) == 0
    row = lax.broadcasted_iota(jnp.int32, (32, 128), 0)
    col = lax.broadcasted_iota(jnp.int32, (32, 128), 1)
    pm = jnp.where((row & 1) == 0, 1.0, -1.0)
    eye = [jnp.where(row + 32 * k == col, BOOST, 0.0).astype(BF16) for k in (0, 2, 1, 3)]
    eye_pm = [jnp.where(row + 32 * k == col, pm, 0.0).astype(BF16) for k in range(4)]
    tab[0] = jnp.full((64, 128), -jnp.inf, F32)
    tab[1] = jnp.full((64, 128), -jnp.inf, F32)
    tab[4] = jnp.full((64, 128), jnp.inf, F32)
    tab[5] = jnp.full((64, 128), jnp.inf, F32)

    @pl.when(me == 2)
    def _():
        pl.semaphore_wait(bar, 3)
        for dst in (0, 1, 3):
            signal(go, dst)

    cp_in.wait()
    xf = jnp.clip(xv[...], -BF16_MAX, BF16_MAX)
    t = _transpose(jnp.concatenate([xf, xf], axis=0).astype(BF16), eye_pm)
    y = [None] * 16
    for a, wire in zip(_ARRIVAL, _WIRES):
        y[wire] = t[a]
    for layer in _NET16:
        for a, b in layer:
            y[a], y[b] = mx(y[a], y[b]), mn(y[a], y[b])
    for v in range(8):
        a, pb = y[v], _roll(y[15 - v], 4)
        hi, lo = mx(a, pb), mn(a, pb)
        y[v] = jnp.where(low[4], hi, lo)
        y[15 - v] = _roll(jnp.where(low[4], lo, hi), 4)
    for bit in (8, 4, 2, 1):
        y = _vstage(y, bit, mx, mn)
    t = list(y)
    for v in range(0, 16, 2):
        u = jnp.where(low[2], t[v], _roll(t[v + 1], 2))
        w = jnp.where(low[2], _roll(t[15 - v], 2), _roll(t[14 - v], 4))
        y[v], y[v + 1] = mx(u, w), mn(u, w)
    y = _xstage(y, 4, 1, low, mx, mn)
    for bit in (8, 4, 2):
        y = _vstage(y, bit, mx, mn)
    y = _xstage(y, 2, 2, low, mx, mn)
    ua, ub = [], []
    for v in (0, 1, 4, 5, 8, 9, 12, 13):
        u, w = _split(y[v], y[v + 2], 1, low)
        ua.append(u)
        ub.append(-w)

    def finish_half(h, half):
        h = [_sstage(r, 4, low, mx, mn) for r in h]
        for bit in (1, 4, 2):
            h = _vstage(h, bit, mx, mn)
        h = _xstage(h, 2, 1, low, mx, mn)
        h = _xstage(h, 1, 4, low, mx, mn)
        dn = [jnp.where(lane_lo, h[q], h[q + 4]) for q in range(4)]
        for q in range(2):
            w = pltpu.bitcast(dn[2 * q + 1], U32) | (pltpu.bitcast(dn[2 * q], U32) >> 16)
            sbuf[half, pl.ds(q, 8, stride=2), :] = w
        return h

    def copy(k, slot, dst, src=sbuf):
        return pltpu.make_async_remote_copy(
            src_ref=src, dst_ref=rbuf.at[slot], send_sem=ssem.at[k],
            recv_sem=rsem.at[slot], device_id=(dst,), device_id_type=MESH)

    head = pltpu.make_async_remote_copy(
        src_ref=sbuf.at[1, pl.ds(SKIP, 16 - SKIP)],
        dst_ref=fbuf.at[pl.ds(SKIP, 16 - SKIP)], send_sem=ssem.at[2],
        recv_sem=rsem.at[3], device_id=(0,), device_id_type=MESH)

    h_lo = finish_half([mn(a, b) for a, b in zip(ua, ub)], 1)

    @pl.when(me == 2)
    def _():
        head.start()

    h_hi = finish_half([mx(a, b) for a, b in zip(ua, ub)], 0)

    @pl.when(me == 2)
    def _():
        copy(0, 1, 3).start()
        copy(1, 1, 1).start()

    @pl.when((me & 1) == 1)
    def _():
        pl.semaphore_wait(bar, 1)
        copy(0, me >> 1, 0).start()
        pl.semaphore_wait(go, 1)
        copy(2, 2, 4 - me).start()
        copy(1, me >> 1, 2).start()

    @pl.when(me == 0)
    def _():
        pl.semaphore_wait(bar, 2)
        copy(0, 0, 1).start()
        copy(1, 0, 3).start()
        pl.semaphore_wait(go, 1)
        copy(2, 2, 2).start()

    for half, h in ((0, h_hi), (1, h_lo)):
        for q in range(4):
            own[half, pl.ds(3 - q, 8, stride=4), :] = jnp.where(lane_lo, h[q + 4], h[q])
    ow = [_roll(own[(7 - k) // 4, pl.ds(8 * ((7 - k) % 4), 8), :], 4) for k in range(8)]

    def clean6(z, bits=(4, 2, 1)):
        for bit in bits:
            z = _vstage(z, bit, mn, mx)
        for d in (4, 2, 1):
            z = [_sstage(r, d, low, mn, mx) for r in z]
        return z

    def clean7(z):
        z = clean6(z)
        r = [pltpu.roll(a, 64, axis=1) for a in z]
        return [jnp.where(lane_lo, mn(a, b), mx(a, b)) for a, b in zip(z, r)]

    def emit(z, bits=(4, 2, 1)):
        ws = []
        for r in clean6(z, bits):
            w = pltpu.bitcast(r, U32)
            ws.append(pltpu.bitcast(w | (w >> 16), BF16))
        e = _transpose(jnp.concatenate(ws, axis=0), eye)
        for k in range(8):
            e0, e1 = e[k + (k & 4)], e[k + (k & 4) + 4]
            r = jnp.where(lane_even, mn(e0, e1), mx(e0, e1))
            o_ref[pl.ds(8 * k, 8), :] = r * (1.0 / BOOST)

    def block(ref):
        return [ref[pl.ds(8 * k, 8), :] for k in range(8)]

    copy(0, 0, me).wait_recv()
    n1 = _load_list(rbuf.at[0])
    b0 = clean7([mn(a, b) for a, b in zip(ow, n1)])
    b1 = clean7([mx(a, b) for a, b in zip(ow, n1)])
    for k in range(8):
        tab[2, pl.ds(8 * k, 8), :] = b0[k]
        tab[3, pl.ds(8 * k, 8), :] = b1[k]
    copy(0, 1, me).wait_recv()
    n2 = _load_list(rbuf.at[1])
    ta, tb, tc = block(tab.at[me]), block(tab.at[me + 1]), block(tab.at[me + 2])
    s_lo = clean7([mn(mx(u, a), b) for u, a, b in zip(n2, ta, tb)])
    s_hi = clean7([mn(mx(u, a), b) for u, a, b in zip(n2, tb, tc)])

    for k in range(2):
        copy(k, 0, me).wait_send()

    @pl.when(me == 2)
    def _():
        head.wait_send()

    @pl.when(me != 2)
    def _():
        copy(2, 0, me).wait_send()

    def head_too_short(u4, s4):
        hit = jnp.logical_and(u4 < s4, sub == 2 * SKIP)
        return jnp.max(jnp.where(hit, 1.0, 0.0)) > 0.0

    def full():
        copy(0, 2, me).wait_recv()
        u = _load_list(rbuf.at[2])
        emit([mn(mx(r, a), b) for r, a, b in zip(u, s_lo, s_hi)])
        return u

    @pl.when(me != 0)
    def _():
        u = full()

        @pl.when(me == 1)
        def _():
            s0 = clean7([mn(r, b) for r, b in zip(u, block(tab.at[2]))])

            @pl.when(head_too_short(_load_half(rbuf.at[1, 1])[0], s0[4]))
            def _():
                fwd = copy(2, 2, 0, rbuf.at[1])
                fwd.start()
                fwd.wait_send()

    @pl.when(me == 0)
    def _():
        head.wait_recv()
        ul = _load_half(fbuf)
        redo = head_too_short(ul[0], s_hi[4])
        z = [mn(r, a) for r, a in zip(ul, s_hi[:4])]
        z += [mx(a, mn(r, b)) for r, a, b in zip(ul, s_hi[:4], s_hi[4:])]
        emit(z, (2, 1))

        @pl.when(redo)
        def _():
            full()


def _compiler_params():
    try:
        return pltpu.CompilerParams(collective_id=0, disable_semaphore_checks=True)
    except TypeError:
        return pltpu.CompilerParams(collective_id=0)


def pallas_dist_sort_i_m128_n64_kernel(x: jax.Array):
    out = pl.pallas_call(
        _body,
        out_shape=jax.ShapeDtypeStruct((64, 128), F32),
        in_specs=[pl.BlockSpec(memory_space=pl.ANY)],
        out_specs=pl.BlockSpec(memory_space=pltpu.VMEM),
        scratch_shapes=[
            pltpu.VMEM((64, 128), F32),
            pltpu.VMEM((2, 16, 128), U32),
            pltpu.VMEM((3, 2, 16, 128), U32),
            pltpu.VMEM((16, 128), U32),
            pltpu.VMEM((2, 32, 128), F32),
            pltpu.VMEM((6, 64, 128), F32),
            pltpu.SemaphoreType.DMA,
            pltpu.SemaphoreType.DMA((3,)),
            pltpu.SemaphoreType.DMA((4,)),
            pltpu.SemaphoreType.REGULAR,
        ],
        compiler_params=_compiler_params(),
    )(x.T)
    return out.T
```

```python
import jax
import jax.numpy as jnp
from jax import lax
from jax.experimental import pallas as pl
from jax.experimental.pallas import tpu as pltpu

F32 = jnp.float32
BF16 = jnp.bfloat16
U32 = jnp.uint32
MESH = pl.DeviceIdType.MESH

EARLY = 19

BF16_MAX = 3.3895313892515355e38
BOOST = 1.0078125

_NET16 = (
    ((0, 13), (1, 12), (2, 15), (3, 14), (4, 8), (5, 6), (7, 11), (9, 10)),
    ((0, 5), (1, 7), (2, 9), (3, 4), (6, 13), (8, 14), (10, 15), (11, 12)),
    ((0, 1), (2, 3), (4, 5), (6, 8), (7, 9), (10, 11), (12, 13), (14, 15)),
    ((0, 2), (1, 3), (4, 10), (5, 11), (6, 7), (8, 9), (12, 14), (13, 15)),
    ((1, 2), (3, 12), (4, 6), (5, 7), (8, 10), (9, 11), (13, 14)),
    ((1, 4), (2, 6), (5, 8), (7, 10), (9, 13), (11, 14)),
    ((2, 4), (3, 6), (9, 12), (11, 13)),
    ((3, 5), (6, 8), (7, 9), (10, 12)),
    ((3, 4), (5, 6), (7, 8), (9, 10), (11, 12)),
    ((6, 7), (8, 9)),
)
_ARRIVAL = (0, 4, 8, 12, 1, 5, 9, 13, 2, 6, 10, 14, 3, 7, 11, 15)
_WIRES = (0, 13, 5, 6, 1, 12, 7, 11, 2, 15, 9, 10, 3, 14, 4, 8)


def _roll(x, s):
    return pltpu.roll(x, s, axis=0)


def _vstage(y, bit, first, second):
    out = list(y)
    for v in range(len(y)):
        if not v & bit:
            out[v] = first(y[v], y[v | bit])
            out[v | bit] = second(y[v], y[v | bit])
    return out


def _sstage(x, d, low, first, second):
    if d == 4:
        r = _roll(x, 4)
        return jnp.where(low[4], first(x, r), second(x, r))
    return jnp.where(low[d], first(x, _roll(x, 8 - d)), second(x, _roll(x, d)))


def _split(a, b, d, low):
    if d == 4:
        return jnp.where(low[4], a, b), _roll(jnp.where(low[4], b, a), 4)
    return jnp.where(low[d], a, _roll(b, d)), jnp.where(low[d], _roll(a, 8 - d), b)


def _xstage(y, d, bit, low, first, second):
    out = list(y)
    for v in range(len(y)):
        if not v & bit:
            u, w = _split(y[v], y[v | bit], d, low)
            out[v] = first(u, w)
            out[v | bit] = second(u, w)
    return out


def _transpose(w, lhs):
    out = []
    for blk in lhs:
        p = lax.dot_general(blk, w, (((1,), (1,)), ((), ())), preferred_element_type=F32)
        out += [p[8 * j:8 * j + 8, :] for j in range(4)]
    return out


def _load_list(ref):
    out = []
    for m in range(4):
        t = pltpu.bitcast(ref[m // 2, pl.ds(8 * (m % 2), 8), :], BF16).astype(F32)
        out += [t[0:8], t[8:16]]
    return out


def _body(x_hbm, o_ref, xv, sbuf, rbuf, fbuf, raw, own, tab, in_sem, ssem, rsem, go):
    me = lax.axis_index("i")
    cp_in = pltpu.make_async_copy(x_hbm, xv, in_sem)
    cp_in.start()

    bar = pltpu.get_barrier_semaphore()

    def signal(sem, dst):
        pl.semaphore_signal(sem, inc=1, device_id=(dst,), device_id_type=MESH)

    @pl.when(me == 0)
    def _():
        for dst in (2, 1, 3):
            signal(bar, dst)

    @pl.when((me & 1) == 1)
    def _():
        for dst in (2, 0):
            signal(bar, dst)

    mx, mn = jnp.maximum, jnp.minimum
    sub = lax.broadcasted_iota(jnp.int32, (8, 128), 0)
    lane = lax.broadcasted_iota(jnp.int32, (8, 128), 1)
    low = {d: (sub & d) == 0 for d in (1, 2, 4)}
    lane_lo = lane < 64
    lane_even = (lane & 1) == 0
    row = lax.broadcasted_iota(jnp.int32, (32, 128), 0)
    col = lax.broadcasted_iota(jnp.int32, (32, 128), 1)
    pm = jnp.where((row & 1) == 0, 1.0, -1.0)
    eye = [jnp.where(row + 32 * k == col, BOOST, 0.0).astype(BF16) for k in (0, 2, 1, 3)]
    eye_pm = [jnp.where(row + 32 * k == col, pm, 0.0).astype(BF16) for k in range(4)]
    tab[0] = jnp.full((64, 128), -jnp.inf, F32)
    tab[1] = jnp.full((64, 128), -jnp.inf, F32)
    tab[4] = jnp.full((64, 128), jnp.inf, F32)
    tab[5] = jnp.full((64, 128), jnp.inf, F32)

    @pl.when(me == 2)
    def _():
        pl.semaphore_wait(bar, 3)
        for dst in (0, 1, 3):
            signal(go, dst)

    def presort(w):
        t = _transpose(w, eye_pm)
        y = [None] * 16
        for a, wire in zip(_ARRIVAL, _WIRES):
            y[wire] = t[a]
        for layer in _NET16:
            for a, b in layer:
                y[a], y[b] = mx(y[a], y[b]), mn(y[a], y[b])
        for v in range(8):
            a, pb = y[v], _roll(y[15 - v], 4)
            hi, lo = mx(a, pb), mn(a, pb)
            y[v] = jnp.where(low[4], hi, lo)
            y[15 - v] = _roll(jnp.where(low[4], lo, hi), 4)
        for bit in (8, 4, 2, 1):
            y = _vstage(y, bit, mx, mn)
        t = list(y)
        for v in range(0, 16, 2):
            u = jnp.where(low[2], t[v], _roll(t[v + 1], 2))
            w = jnp.where(low[2], _roll(t[15 - v], 2), _roll(t[14 - v], 4))
            y[v], y[v + 1] = mx(u, w), mn(u, w)
        y = _xstage(y, 4, 1, low, mx, mn)
        for bit in (8, 4, 2):
            y = _vstage(y, bit, mx, mn)
        y = _xstage(y, 2, 2, low, mx, mn)
        ua, ub = [], []
        for v in (0, 1, 4, 5, 8, 9, 12, 13):
            u, w = _split(y[v], y[v + 2], 1, low)
            ua.append(u)
            ub.append(-w)
        return ua, ub

    def finish_half(h, dst):
        h = [_sstage(r, 4, low, mx, mn) for r in h]
        for bit in (1, 4, 2):
            h = _vstage(h, bit, mx, mn)
        h = _xstage(h, 2, 1, low, mx, mn)
        h = _xstage(h, 1, 4, low, mx, mn)
        dn = [jnp.where(lane_lo, h[q], h[q + 4]) for q in range(4)]
        for q in range(2):
            w = pltpu.bitcast(dn[2 * q + 1], U32) | (pltpu.bitcast(dn[2 * q], U32) >> 16)
            dst[pl.ds(q, 8, stride=2), :] = w
        return h

    def copy(k, slot, dst):
        return pltpu.make_async_remote_copy(
            src_ref=sbuf, dst_ref=rbuf.at[slot], send_sem=ssem.at[k],
            recv_sem=rsem.at[slot], device_id=(dst,), device_id_type=MESH)

    head = pltpu.make_async_remote_copy(
        src_ref=sbuf.at[1, pl.ds(4, 12)], dst_ref=fbuf, send_sem=ssem.at[2],
        recv_sem=rsem.at[3], device_id=(0,), device_id_type=MESH)

    def backup(part):
        rows = pl.ds(EARLY, 32 - EARLY) if part else pl.ds(0, EARLY)
        return pltpu.make_async_remote_copy(
            src_ref=raw.at[0, rows], dst_ref=raw.at[1, rows], send_sem=ssem.at[3 + part],
            recv_sem=rsem.at[4 + part], device_id=(0,), device_id_type=MESH)

    cp_in.wait()
    xf = jnp.clip(xv[...], -BF16_MAX, BF16_MAX)
    raw[0] = pltpu.bitcast(xf.astype(BF16), U32)

    @pl.when(me == 2)
    def _():
        backup(0).start()

    ua, ub = presort(jnp.concatenate([xf, xf], axis=0).astype(BF16))
    h_lo = finish_half([mn(a, b) for a, b in zip(ua, ub)], sbuf.at[1])

    @pl.when(me == 2)
    def _():
        head.start()
        backup(1).start()

    h_hi = finish_half([mx(a, b) for a, b in zip(ua, ub)], sbuf.at[0])

    @pl.when(me == 2)
    def _():
        copy(0, 1, 3).start()
        copy(1, 1, 1).start()

    @pl.when((me & 1) == 1)
    def _():
        pl.semaphore_wait(bar, 1)
        copy(0, me >> 1, 0).start()
        pl.semaphore_wait(go, 1)
        copy(2, 2, 4 - me).start()
        copy(1, me >> 1, 2).start()

    @pl.when(me == 0)
    def _():
        pl.semaphore_wait(bar, 2)
        copy(0, 0, 1).start()
        copy(1, 0, 3).start()
        pl.semaphore_wait(go, 1)
        copy(2, 2, 2).start()

    for half, h in ((0, h_hi), (1, h_lo)):
        for q in range(4):
            own[half, pl.ds(3 - q, 8, stride=4), :] = jnp.where(lane_lo, h[q + 4], h[q])
    ow = [_roll(own[(7 - k) // 4, pl.ds(8 * ((7 - k) % 4), 8), :], 4) for k in range(8)]

    def clean6(z, bits=(4, 2, 1)):
        for bit in bits:
            z = _vstage(z, bit, mn, mx)
        for d in (4, 2, 1):
            z = [_sstage(r, d, low, mn, mx) for r in z]
        return z

    def clean7(z):
        z = clean6(z)
        r = [pltpu.roll(a, 64, axis=1) for a in z]
        return [jnp.where(lane_lo, mn(a, b), mx(a, b)) for a, b in zip(z, r)]

    def emit(z, bits=(4, 2, 1)):
        ws = []
        for r in clean6(z, bits):
            w = pltpu.bitcast(r, U32)
            ws.append(pltpu.bitcast(w | (w >> 16), BF16))
        e = _transpose(jnp.concatenate(ws, axis=0), eye)
        for k in range(8):
            e0, e1 = e[k + (k & 4)], e[k + (k & 4) + 4]
            r = jnp.where(lane_even, mn(e0, e1), mx(e0, e1))
            o_ref[pl.ds(8 * k, 8), :] = r * (1.0 / BOOST)

    def block(ref):
        return [ref[pl.ds(8 * k, 8), :] for k in range(8)]

    copy(0, 0, me).wait_recv()
    n1 = _load_list(rbuf.at[0])
    b0 = clean7([mn(a, b) for a, b in zip(ow, n1)])
    b1 = clean7([mx(a, b) for a, b in zip(ow, n1)])
    for k in range(8):
        tab[2, pl.ds(8 * k, 8), :] = b0[k]
        tab[3, pl.ds(8 * k, 8), :] = b1[k]
    copy(0, 1, me).wait_recv()
    n2 = _load_list(rbuf.at[1])
    ta, tb, tc = block(tab.at[me]), block(tab.at[me + 1]), block(tab.at[me + 2])
    s_lo = clean7([mn(mx(u, a), b) for u, a, b in zip(n2, ta, tb)])
    s_hi = clean7([mn(mx(u, a), b) for u, a, b in zip(n2, tb, tc)])

    for k in range(2):
        copy(k, 0, me).wait_send()

    @pl.when(me == 2)
    def _():
        head.wait_send()
        backup(0).wait_send()
        backup(1).wait_send()

    @pl.when(me != 2)
    def _():
        copy(2, 0, me).wait_send()

    def full():
        u = _load_list(rbuf.at[2])
        emit([mn(mx(r, a), b) for r, a, b in zip(u, s_lo, s_hi)])

    @pl.when(me != 0)
    def _():
        copy(0, 2, me).wait_recv()
        full()

    @pl.when(me == 0)
    def _():
        backup(0).wait_recv()
        head.wait_recv()
        t = pltpu.bitcast(fbuf[pl.ds(0, 8), :], BF16).astype(F32)
        ul = [t[0:8], t[8:16], pltpu.bitcast(fbuf[pl.ds(8, 4), :], BF16).astype(F32)]
        hit = jnp.logical_and(ul[0] < s_hi[5], jnp.logical_and(sub == 0, lane_lo))
        redo = jnp.max(jnp.where(hit, 1.0, 0.0)) > 0.0
        z = [s_hi[0]] + [mn(r, a) for r, a in zip(ul, s_hi[1:4])]
        z += [s_hi[4]] + [mx(a, mn(r, b)) for r, a, b in zip(ul, s_hi[1:4], s_hi[5:])]
        emit(z, (2, 1))

        @pl.when(redo)
        def _():
            backup(1).wait_recv()
            g = raw[1]
            va, vb = presort(pltpu.bitcast(jnp.concatenate([g, g], axis=0), BF16))
            finish_half([mn(a, b) for a, b in zip(va, vb)], rbuf.at[2, 1])
            finish_half([mx(a, b) for a, b in zip(va, vb)], rbuf.at[2, 0])
            full()

        @pl.when(jnp.logical_not(redo))
        def _():
            backup(1).wait_recv()


def _compiler_params():
    try:
        return pltpu.CompilerParams(collective_id=0, disable_semaphore_checks=True)
    except TypeError:
        return pltpu.CompilerParams(collective_id=0)


def pallas_dist_sort_i_m128_n64_kernel(x: jax.Array):
    out = pl.pallas_call(
        _body,
        out_shape=jax.ShapeDtypeStruct((64, 128), F32),
        in_specs=[pl.BlockSpec(memory_space=pl.ANY)],
        out_specs=pl.BlockSpec(memory_space=pltpu.VMEM),
        scratch_shapes=[
            pltpu.VMEM((64, 128), F32),
            pltpu.VMEM((2, 16, 128), U32),
            pltpu.VMEM((3, 2, 16, 128), U32),
            pltpu.VMEM((12, 128), U32),
            pltpu.VMEM((2, 32, 128), U32),
            pltpu.VMEM((2, 32, 128), F32),
            pltpu.VMEM((6, 64, 128), F32),
            pltpu.SemaphoreType.DMA,
            pltpu.SemaphoreType.DMA((5,)),
            pltpu.SemaphoreType.DMA((6,)),
            pltpu.SemaphoreType.REGULAR,
        ],
        compiler_params=_compiler_params(),
    )(x.T)
    return out.T
```

```python
import jax
import jax.numpy as jnp
from jax import lax
from jax.experimental import pallas as pl
from jax.experimental.pallas import tpu as pltpu

F32 = jnp.float32
BF16 = jnp.bfloat16
U32 = jnp.uint32
MESH = pl.DeviceIdType.MESH

EARLY = 19

BF16_MAX = 3.3895313892515355e38
BOOST = 1.0078125

_NET16 = (
    ((0, 13), (1, 12), (2, 15), (3, 14), (4, 8), (5, 6), (7, 11), (9, 10)),
    ((0, 5), (1, 7), (2, 9), (3, 4), (6, 13), (8, 14), (10, 15), (11, 12)),
    ((0, 1), (2, 3), (4, 5), (6, 8), (7, 9), (10, 11), (12, 13), (14, 15)),
    ((0, 2), (1, 3), (4, 10), (5, 11), (6, 7), (8, 9), (12, 14), (13, 15)),
    ((1, 2), (3, 12), (4, 6), (5, 7), (8, 10), (9, 11), (13, 14)),
    ((1, 4), (2, 6), (5, 8), (7, 10), (9, 13), (11, 14)),
    ((2, 4), (3, 6), (9, 12), (11, 13)),
    ((3, 5), (6, 8), (7, 9), (10, 12)),
    ((3, 4), (5, 6), (7, 8), (9, 10), (11, 12)),
    ((6, 7), (8, 9)),
)
_ARRIVAL = (0, 4, 8, 12, 1, 5, 9, 13, 2, 6, 10, 14, 3, 7, 11, 15)
_WIRES = (0, 13, 5, 6, 1, 12, 7, 11, 2, 15, 9, 10, 3, 14, 4, 8)


def _roll(x, s):
    return pltpu.roll(x, s, axis=0)


def _vstage(y, bit, first, second):
    out = list(y)
    for v in range(len(y)):
        if not v & bit:
            out[v] = first(y[v], y[v | bit])
            out[v | bit] = second(y[v], y[v | bit])
    return out


def _sstage(x, d, low, first, second):
    if d == 4:
        r = _roll(x, 4)
        return jnp.where(low[4], first(x, r), second(x, r))
    return jnp.where(low[d], first(x, _roll(x, 8 - d)), second(x, _roll(x, d)))


def _split(a, b, d, low):
    if d == 4:
        return jnp.where(low[4], a, b), _roll(jnp.where(low[4], b, a), 4)
    return jnp.where(low[d], a, _roll(b, d)), jnp.where(low[d], _roll(a, 8 - d), b)


def _xstage(y, d, bit, low, first, second):
    out = list(y)
    for v in range(len(y)):
        if not v & bit:
            u, w = _split(y[v], y[v | bit], d, low)
            out[v] = first(u, w)
            out[v | bit] = second(u, w)
    return out


def _transpose(w, lhs):
    out = []
    for blk in lhs:
        p = lax.dot_general(blk, w, (((1,), (1,)), ((), ())), preferred_element_type=F32)
        out += [p[8 * j:8 * j + 8, :] for j in range(4)]
    return out


def _load_list(ref):
    out = []
    for m in range(4):
        t = pltpu.bitcast(ref[m // 2, pl.ds(8 * (m % 2), 8), :], BF16).astype(F32)
        out += [t[0:8], t[8:16]]
    return out


def _body(x_hbm, o_ref, xv, sbuf, rbuf, fbuf, raw, own, tab, in_sem, ssem, rsem, go):
    me = lax.axis_index("i")
    cp_in = pltpu.make_async_copy(x_hbm, xv, in_sem)
    cp_in.start()

    bar = pltpu.get_barrier_semaphore()

    def signal(sem, dst):
        pl.semaphore_signal(sem, inc=1, device_id=(dst,), device_id_type=MESH)

    @pl.when(me == 0)
    def _():
        for dst in (2, 1, 3):
            signal(bar, dst)

    @pl.when((me & 1) == 1)
    def _():
        for dst in (2, 0):
            signal(bar, dst)

    mx, mn = jnp.maximum, jnp.minimum
    sub = lax.broadcasted_iota(jnp.int32, (8, 128), 0)
    lane = lax.broadcasted_iota(jnp.int32, (8, 128), 1)
    low = {d: (sub & d) == 0 for d in (1, 2, 4)}
    lane_lo = lane < 64
    lane_even = (lane & 1) == 0
    row = lax.broadcasted_iota(jnp.int32, (32, 128), 0)
    col = lax.broadcasted_iota(jnp.int32, (32, 128), 1)
    pm = jnp.where((row & 1) == 0, 1.0, -1.0)
    eye = [jnp.where(row + 32 * k == col, BOOST, 0.0).astype(BF16) for k in (0, 2, 1, 3)]
    eye_pm = [jnp.where(row + 32 * k == col, pm, 0.0).astype(BF16) for k in range(4)]
    tab[0] = jnp.full((64, 128), -jnp.inf, F32)
    tab[1] = jnp.full((64, 128), -jnp.inf, F32)
    tab[4] = jnp.full((64, 128), jnp.inf, F32)
    tab[5] = jnp.full((64, 128), jnp.inf, F32)

    @pl.when(me == 2)
    def _():
        pl.semaphore_wait(bar, 3)
        for dst in (0, 1, 3):
            signal(go, dst)

    def presort(w):
        t = _transpose(w, eye_pm)
        y = [None] * 16
        for a, wire in zip(_ARRIVAL, _WIRES):
            y[wire] = t[a]
        for layer in _NET16:
            for a, b in layer:
                y[a], y[b] = mx(y[a], y[b]), mn(y[a], y[b])
        for v in range(8):
            a, pb = y[v], _roll(y[15 - v], 4)
            hi, lo = mx(a, pb), mn(a, pb)
            y[v] = jnp.where(low[4], hi, lo)
            y[15 - v] = _roll(jnp.where(low[4], lo, hi), 4)
        for bit in (8, 4, 2, 1):
            y = _vstage(y, bit, mx, mn)
        t = list(y)
        for v in range(0, 16, 2):
            u = jnp.where(low[2], t[v], _roll(t[v + 1], 2))
            w = jnp.where(low[2], _roll(t[15 - v], 2), _roll(t[14 - v], 4))
            y[v], y[v + 1] = mx(u, w), mn(u, w)
        y = _xstage(y, 4, 1, low, mx, mn)
        for bit in (8, 4, 2):
            y = _vstage(y, bit, mx, mn)
        y = _xstage(y, 2, 2, low, mx, mn)
        ua, ub = [], []
        for v in (0, 1, 4, 5, 8, 9, 12, 13):
            u, w = _split(y[v], y[v + 2], 1, low)
            ua.append(u)
            ub.append(-w)
        return ua, ub

    def finish_half(h, dst):
        h = [_sstage(r, 4, low, mx, mn) for r in h]
        for bit in (1, 4, 2):
            h = _vstage(h, bit, mx, mn)
        h = _xstage(h, 2, 1, low, mx, mn)
        h = _xstage(h, 1, 4, low, mx, mn)
        dn = [jnp.where(lane_lo, h[q], h[q + 4]) for q in range(4)]
        for q in range(2):
            w = pltpu.bitcast(dn[2 * q + 1], U32) | (pltpu.bitcast(dn[2 * q], U32) >> 16)
            dst[pl.ds(q, 8, stride=2), :] = w
        return h

    def copy(k, slot, dst):
        return pltpu.make_async_remote_copy(
            src_ref=sbuf, dst_ref=rbuf.at[slot], send_sem=ssem.at[k],
            recv_sem=rsem.at[slot], device_id=(dst,), device_id_type=MESH)

    head = pltpu.make_async_remote_copy(
        src_ref=sbuf.at[1, pl.ds(4, 12)], dst_ref=fbuf, send_sem=ssem.at[2],
        recv_sem=rsem.at[3], device_id=(0,), device_id_type=MESH)

    def backup(part):
        rows = pl.ds(EARLY, 32 - EARLY) if part else pl.ds(0, EARLY)
        return pltpu.make_async_remote_copy(
            src_ref=raw.at[0, rows], dst_ref=raw.at[1, rows], send_sem=ssem.at[3 + part],
            recv_sem=rsem.at[4 + part], device_id=(0,), device_id_type=MESH)

    cp_in.wait()
    xf = jnp.clip(xv[...], -BF16_MAX, BF16_MAX)
    raw[0] = pltpu.bitcast(xf.astype(BF16), U32)

    @pl.when(me == 2)
    def _():
        backup(0).start()

    ua, ub = presort(jnp.concatenate([xf, xf], axis=0).astype(BF16))
    h_lo = finish_half([mn(a, b) for a, b in zip(ua, ub)], sbuf.at[1])

    @pl.when(me == 2)
    def _():
        head.start()
        backup(1).start()

    h_hi = finish_half([mx(a, b) for a, b in zip(ua, ub)], sbuf.at[0])

    @pl.when(me == 2)
    def _():
        copy(0, 1, 3).start()
        copy(1, 1, 1).start()

    for odd in (1, 3):
        @pl.when(me == odd)
        def _():
            pl.semaphore_wait(bar, 1)
            copy(0, odd // 2, 0).start()
            pl.semaphore_wait(go, 1)
            copy(2, 2, 4 - odd).start()
            copy(1, odd // 2, 2).start()

    @pl.when(me == 0)
    def _():
        pl.semaphore_wait(bar, 2)
        copy(0, 0, 1).start()
        copy(1, 0, 3).start()
        pl.semaphore_wait(go, 1)
        copy(2, 2, 2).start()

    for half, h in ((0, h_hi), (1, h_lo)):
        for q in range(4):
            own[half, pl.ds(3 - q, 8, stride=4), :] = jnp.where(lane_lo, h[q + 4], h[q])
    ow = [_roll(own[(7 - k) // 4, pl.ds(8 * ((7 - k) % 4), 8), :], 4) for k in range(8)]

    def clean6(z, bits=(4, 2, 1)):
        for bit in bits:
            z = _vstage(z, bit, mn, mx)
        for d in (4, 2, 1):
            z = [_sstage(r, d, low, mn, mx) for r in z]
        return z

    def clean7(z):
        z = clean6(z)
        r = [pltpu.roll(a, 64, axis=1) for a in z]
        return [jnp.where(lane_lo, mn(a, b), mx(a, b)) for a, b in zip(z, r)]

    def emit(z, bits=(4, 2, 1)):
        ws = []
        for r in clean6(z, bits):
            w = pltpu.bitcast(r, U32)
            ws.append(pltpu.bitcast(w | (w >> 16), BF16))
        e = _transpose(jnp.concatenate(ws, axis=0), eye)
        for k in range(8):
            e0, e1 = e[k + (k & 4)], e[k + (k & 4) + 4]
            r = jnp.where(lane_even, mn(e0, e1), mx(e0, e1))
            o_ref[pl.ds(8 * k, 8), :] = r * (1.0 / BOOST)

    def block(ref):
        return [ref[pl.ds(8 * k, 8), :] for k in range(8)]

    copy(0, 0, me).wait_recv()
    n1 = _load_list(rbuf.at[0])
    b0 = clean7([mn(a, b) for a, b in zip(ow, n1)])
    b1 = clean7([mx(a, b) for a, b in zip(ow, n1)])
    for k in range(8):
        tab[2, pl.ds(8 * k, 8), :] = b0[k]
        tab[3, pl.ds(8 * k, 8), :] = b1[k]
    copy(0, 1, me).wait_recv()
    n2 = _load_list(rbuf.at[1])
    ta, tb, tc = block(tab.at[me]), block(tab.at[me + 1]), block(tab.at[me + 2])
    s_lo = clean7([mn(mx(u, a), b) for u, a, b in zip(n2, ta, tb)])
    s_hi = clean7([mn(mx(u, a), b) for u, a, b in zip(n2, tb, tc)])

    for k in range(2):
        copy(k, 0, me).wait_send()

    @pl.when(me == 2)
    def _():
        head.wait_send()
        backup(0).wait_send()
        backup(1).wait_send()

    @pl.when(me != 2)
    def _():
        copy(2, 0, me).wait_send()

    def full():
        u = _load_list(rbuf.at[2])
        emit([mn(mx(r, a), b) for r, a, b in zip(u, s_lo, s_hi)])

    @pl.when(me != 0)
    def _():
        copy(0, 2, me).wait_recv()
        full()

    @pl.when(me == 0)
    def _():
        backup(0).wait_recv()
        head.wait_recv()
        t = pltpu.bitcast(fbuf[pl.ds(0, 8), :], BF16).astype(F32)
        ul = [t[0:8], t[8:16], pltpu.bitcast(fbuf[pl.ds(8, 4), :], BF16).astype(F32)]
        hit = jnp.logical_and(ul[0] < s_hi[5], jnp.logical_and(sub == 0, lane_lo))
        redo = jnp.max(jnp.where(hit, 1.0, 0.0)) > 0.0
        z = [s_hi[0]] + [mn(r, a) for r, a in zip(ul, s_hi[1:4])]
        z += [s_hi[4]] + [mx(a, mn(r, b)) for r, a, b in zip(ul, s_hi[1:4], s_hi[5:])]
        emit(z, (2, 1))

        @pl.when(redo)
        def _():
            backup(1).wait_recv()
            g = raw[1]
            va, vb = presort(pltpu.bitcast(jnp.concatenate([g, g], axis=0), BF16))
            finish_half([mn(a, b) for a, b in zip(va, vb)], rbuf.at[2, 1])
            finish_half([mx(a, b) for a, b in zip(va, vb)], rbuf.at[2, 0])
            full()

        @pl.when(jnp.logical_not(redo))
        def _():
            backup(1).wait_recv()


def _compiler_params():
    try:
        return pltpu.CompilerParams(collective_id=0, disable_semaphore_checks=True)
    except TypeError:
        return pltpu.CompilerParams(collective_id=0)


def pallas_dist_sort_i_m128_n64_kernel(x: jax.Array):
    out = pl.pallas_call(
        _body,
        out_shape=jax.ShapeDtypeStruct((64, 128), F32),
        in_specs=[pl.BlockSpec(memory_space=pl.ANY)],
        out_specs=pl.BlockSpec(memory_space=pltpu.VMEM),
        scratch_shapes=[
            pltpu.VMEM((64, 128), F32),
            pltpu.VMEM((2, 16, 128), U32),
            pltpu.VMEM((3, 2, 16, 128), U32),
            pltpu.VMEM((12, 128), U32),
            pltpu.VMEM((2, 32, 128), U32),
            pltpu.VMEM((2, 32, 128), F32),
            pltpu.VMEM((6, 64, 128), F32),
            pltpu.SemaphoreType.DMA,
            pltpu.SemaphoreType.DMA((5,)),
            pltpu.SemaphoreType.DMA((6,)),
            pltpu.SemaphoreType.REGULAR,
        ],
        compiler_params=_compiler_params(),
    )(x.T)
    return out.T
```
